```python
import numpy as np

kernel_name = "dist_mean_ax1_xy_m4096_n1024"

def setup_inputs():
    return {"x": np.random.randn(8192, 2048).astype(np.float32)}

def reference(x: np.ndarray) -> np.ndarray:
    return np.mean(x, axis=1, keepdims=True)
```

```python
import jax
import jax.numpy as jnp
from jax import lax
from jax.experimental import pallas as pl
from jax.experimental.pallas import tpu as pltpu

SUBLANES, LANES = 8, 128
ROWS, COLS = 4096, 1024
Y_SHARDS = 2

CHUNKS = ROWS // SUBLANES
BLOCKS = ROWS // LANES
PER_BLOCK = CHUNKS // BLOCKS

HIGH, LOW = 0, 1
QUEUE_DEPTH = 32
GROUP = 8
TAIL_GROUPS = (8, 6, 2)
LAG = 24
RAMP_CHUNKS = 16
DRAIN_CHUNKS = 4

MESSAGES = (
    tuple(range(0, BLOCKS, 2)),
    tuple(range(1, BLOCKS - 1, 2)),
    (BLOCKS - 1,),
)
LAST_BLOCK_ORDER = (0, 4, 2, 6, 1, 5, 3, 7, 8, 12, 10, 14, 9, 13, 11, 15)


def _read_order():
    order = [
        block * PER_BLOCK + pos
        for blocks in MESSAGES[:-1]
        for pos in range(PER_BLOCK)
        for block in blocks
    ]
    return order + [MESSAGES[-1][0] * PER_BLOCK + pos for pos in LAST_BLOCK_ORDER]


def _pieces(step):
    if step >= CHUNKS - DRAIN_CHUNKS:
        return [(col, LANES, LOW) for col in range(0, COLS, LANES)]
    width = COLS // 2 if step < RAMP_CHUNKS else COLS
    return [
        piece
        for col in range(0, COLS, width)
        for piece in ((col, width - LANES, LOW), (col + width - LANES, LANES, HIGH))
    ]


def _groups():
    body = CHUNKS - sum(TAIL_GROUPS)
    assert body % GROUP == 0
    groups, first = [], 0
    for size in (GROUP,) * (body // GROUP) + TAIL_GROUPS:
        groups.append((first, size))
        first += size
    return groups


def _kernel(x_hbm, out_ref, x_buf, mine, theirs, read_sems, send_sems, recv_sems):
    order = _read_order()
    groups = _groups()
    group_of = [g for g, (_, size) in enumerate(groups) for _ in range(size)]
    queue = {HIGH: [], LOW: []}
    for step in range(CHUNKS):
        for col, width, priority in _pieces(step):
            queue[priority].append((step, col, width))

    def start_read(priority):
        step, col, width = queue[priority].pop(0)
        pltpu.make_async_copy(
            x_hbm.at[order[step], :, pl.ds(col, width)],
            x_buf.at[step, :, pl.ds(col, width)],
            read_sems.at[group_of[step]],
        ).start(priority=priority)

    for _ in range(QUEUE_DEPTH):
        start_read(LOW)

    peer = (lax.axis_index("x"), 1 - lax.axis_index("y"))
    barrier = pltpu.get_barrier_semaphore()
    pl.semaphore_signal(
        barrier, 1, device_id=peer, device_id_type=pl.DeviceIdType.MESH
    )

    def rows_of(m):
        return pl.ds(sum(map(len, MESSAGES[:m])), len(MESSAGES[m]))

    def message(m):
        return pltpu.make_async_remote_copy(
            mine.at[rows_of(m)],
            theirs.at[rows_of(m)],
            send_sems.at[m],
            recv_sems.at[m],
            device_id=peer,
            device_id_type=pl.DeviceIdType.MESH,
        )

    tile = (SUBLANES, LANES)
    diagonal = lax.broadcasted_iota(jnp.int32, tile, 1) - lax.broadcasted_iota(
        jnp.int32, tile, 0
    )
    sums = {block: jnp.zeros(tile, jnp.float32) for block in range(BLOCKS)}
    missing = {block: PER_BLOCK for block in range(BLOCKS)}
    folded = []
    sent = []

    def consume(g):
        first, size = groups[g]
        landed = x_buf.at[pl.ds(first, size)]
        pltpu.make_async_copy(landed, landed, read_sems.at[g]).wait()
        for step in range(first, first + size):
            tiles = [x_buf[step, :, pl.ds(c, LANES)] for c in range(0, COLS, LANES)]
            while len(tiles) > 1:
                tiles = [a + b for a, b in zip(tiles[::2], tiles[1::2])]
            folded.append((order[step], tiles[0]))
        if g == len(groups) - 2:
            return
        while folded:
            chunk, partial = folded.pop(0)
            block, pos = divmod(chunk, PER_BLOCK)
            row_sums = jnp.sum(partial, axis=1, keepdims=True)
            sums[block] = jnp.where(diagonal == pos * SUBLANES, row_sums, sums[block])
            missing[block] -= 1
        for m, blocks in enumerate(MESSAGES):
            if m in sent or any(missing[block] for block in blocks):
                continue
            for i, block in enumerate(blocks):
                row = jnp.sum(sums[block], axis=0, keepdims=True)
                mine[pl.ds(rows_of(m).start + i, 1)] = row * (1.0 / (Y_SHARDS * COLS))
            if not sent:
                pl.semaphore_wait(barrier, 1)
            message(m).start()
            sent.append(m)

    g = 0
    while queue[HIGH] or queue[LOW]:
        for priority in (HIGH, LOW):
            if queue[priority]:
                start_read(priority)
        issued = queue[HIGH][0][0] if queue[HIGH] else CHUNKS - DRAIN_CHUNKS
        if sum(groups[g]) + LAG <= issued:
            consume(g)
            g += 1
    for g in range(g, len(groups)):
        consume(g)

    for m in sent:
        message(m).wait_send()
    for m in sent:
        message(m).wait_recv()
        total = mine[rows_of(m)] + theirs[rows_of(m)]
        for i, block in enumerate(MESSAGES[m]):
            out_ref[pl.ds(block, 1)] = total[i : i + 1]


def pallas_dist_mean_ax1_xy_m4096_n1024_kernel(x: jax.Array):
    assert x.shape == (ROWS, COLS), x.shape
    out = pl.pallas_call(
        _kernel,
        out_shape=jax.ShapeDtypeStruct((BLOCKS, LANES), jnp.float32),
        in_specs=[pl.BlockSpec(memory_space=pl.ANY)],
        out_specs=pl.BlockSpec(memory_space=pltpu.VMEM),
        scratch_shapes=[
            pltpu.VMEM((CHUNKS, SUBLANES, COLS), jnp.float32),
            pltpu.VMEM((BLOCKS, LANES), jnp.float32),
            pltpu.VMEM((BLOCKS, LANES), jnp.float32),
            pltpu.SemaphoreType.DMA((len(_groups()),)),
            pltpu.SemaphoreType.DMA((len(MESSAGES),)),
            pltpu.SemaphoreType.DMA((len(MESSAGES),)),
        ],
        compiler_params=pltpu.CompilerParams(
            collective_id=0,
            vmem_limit_bytes=32 * 1024 * 1024,
            disable_bounds_checks=True,
            disable_semaphore_checks=True,
        ),
    )(x.reshape(CHUNKS, SUBLANES, COLS))
    return out.reshape(ROWS, 1)
```

```python
import jax
import jax.numpy as jnp
from jax import lax
from jax.experimental import pallas as pl
from jax.experimental.pallas import tpu as pltpu

SUBLANES, LANES = 8, 128
ROWS, COLS = 4096, 1024
Y_SHARDS = 2

CHUNKS = ROWS // SUBLANES
BLOCKS = ROWS // LANES
PER_BLOCK = CHUNKS // BLOCKS

HIGH, LOW = 0, 1
QUEUE_DEPTH = 36
RAMP_CHUNKS = 16
GROUP = 8
LAG = 32

MESSAGES = (
    tuple(range(0, BLOCKS, 2)),
    tuple(range(1, BLOCKS - 1, 2)),
    (BLOCKS - 1,),
)
READ_ORDER = tuple(
    block * PER_BLOCK + pos
    for blocks in MESSAGES
    for pos in range(PER_BLOCK)
    for block in blocks
)
GROUPS = (
    *((first, GROUP) for first in range(0, CHUNKS - GROUP, GROUP)),
    (CHUNKS - GROUP, GROUP - 1),
    (CHUNKS - 1, 1),
)


def _copies():
    low, high = [], []
    for step in range(CHUNKS):
        width = COLS // 2 if step < RAMP_CHUNKS else COLS
        for col in range(0, COLS, width):
            low.append((step, col, width - LANES))
            high.append((step, col + width - LANES, LANES))
    return low, high


def _kernel(x_hbm, out_ref, x_buf, mine, theirs, read_sems, send_sems, recv_sems):
    group_of = [g for g, (_, size) in enumerate(GROUPS) for _ in range(size)]
    low, high = _copies()

    def start_read(copies, priority):
        step, col, width = copies.pop(0)
        pltpu.make_async_copy(
            x_hbm.at[READ_ORDER[step], :, pl.ds(col, width)],
            x_buf.at[step, :, pl.ds(col, width)],
            read_sems.at[group_of[step]],
        ).start(priority=priority)

    while len(high) - len(low) < QUEUE_DEPTH:
        start_read(low, LOW)
        start_read(high, HIGH)
        for _ in range(3):
            if len(high) - len(low) < QUEUE_DEPTH:
                start_read(low, LOW)

    peer = (lax.axis_index("x"), 1 - lax.axis_index("y"))
    barrier = pltpu.get_barrier_semaphore()
    pl.semaphore_signal(
        barrier, 1, device_id=peer, device_id_type=pl.DeviceIdType.MESH
    )

    def rows_of(m):
        return pl.ds(sum(map(len, MESSAGES[:m])), len(MESSAGES[m]))

    def message(m):
        return pltpu.make_async_remote_copy(
            mine.at[rows_of(m)],
            theirs.at[rows_of(m)],
            send_sems.at[m],
            recv_sems.at[m],
            device_id=peer,
            device_id_type=pl.DeviceIdType.MESH,
        )

    tile = (SUBLANES, LANES)
    diagonal = lax.broadcasted_iota(jnp.int32, tile, 1) - lax.broadcasted_iota(
        jnp.int32, tile, 0
    )
    sums = [jnp.zeros(tile, jnp.float32)] * BLOCKS
    missing = [PER_BLOCK] * BLOCKS
    folded = []
    sent = []

    def consume(g):
        first, size = GROUPS[g]
        landed = x_buf.at[pl.ds(first, size)]
        pltpu.make_async_copy(landed, landed, read_sems.at[g]).wait()
        rows = landed[...]
        tiles = [rows[:, :, c : c + LANES] for c in range(0, COLS, LANES)]
        while len(tiles) > 1:
            tiles = [a + b for a, b in zip(tiles[::2], tiles[1::2])]
        folded.append((first, tiles[0]))
        if g == len(GROUPS) - 2:
            return
        while folded:
            first, partial = folded.pop(0)
            row_sums = jnp.sum(partial, axis=2, keepdims=True)
            for i in range(partial.shape[0]):
                block, pos = divmod(READ_ORDER[first + i], PER_BLOCK)
                here = diagonal == pos * SUBLANES
                sums[block] = jnp.where(here, row_sums[i], sums[block])
                missing[block] -= 1
        for m, blocks in enumerate(MESSAGES):
            if m in sent or any(missing[block] for block in blocks):
                continue
            for i, block in enumerate(blocks):
                row = jnp.sum(sums[block], axis=0, keepdims=True)
                mine[pl.ds(rows_of(m).start + i, 1)] = row * (1.0 / (Y_SHARDS * COLS))
            if not sent:
                pl.semaphore_wait(barrier, 1)
            message(m).start()
            sent.append(m)

    g = 0
    while high:
        start_read(high, HIGH)
        if low:
            start_read(low, LOW)
        if high and sum(GROUPS[g]) + LAG <= high[0][0]:
            consume(g)
            g += 1
    for g in range(g, len(GROUPS)):
        consume(g)

    for m in sent:
        message(m).wait_send()
    for m in sent:
        message(m).wait_recv()
        total = mine[rows_of(m)] + theirs[rows_of(m)]
        for i, block in enumerate(MESSAGES[m]):
            out_ref[pl.ds(block, 1)] = total[i : i + 1]


def pallas_dist_mean_ax1_xy_m4096_n1024_kernel(x: jax.Array):
    assert x.shape == (ROWS, COLS), x.shape
    out = pl.pallas_call(
        _kernel,
        out_shape=jax.ShapeDtypeStruct((BLOCKS, LANES), jnp.float32),
        in_specs=[pl.BlockSpec(memory_space=pl.ANY)],
        out_specs=pl.BlockSpec(memory_space=pltpu.VMEM),
        scratch_shapes=[
            pltpu.VMEM((CHUNKS, SUBLANES, COLS), jnp.float32),
            pltpu.VMEM((BLOCKS, LANES), jnp.float32),
            pltpu.VMEM((BLOCKS, LANES), jnp.float32),
            pltpu.SemaphoreType.DMA((len(GROUPS),)),
            pltpu.SemaphoreType.DMA((len(MESSAGES),)),
            pltpu.SemaphoreType.DMA((len(MESSAGES),)),
        ],
        compiler_params=pltpu.CompilerParams(
            collective_id=0,
            vmem_limit_bytes=32 * 1024 * 1024,
            disable_bounds_checks=True,
            disable_semaphore_checks=True,
        ),
    )(x.reshape(CHUNKS, SUBLANES, COLS))
    return out.reshape(ROWS, 1)
```
